```python
import numpy as np

kernel_name = "dist_rope_attn_htp_bs_b2_sq512_d1024_hq8_dh128"

def setup_inputs():
    x = np.random.randn(8, 512, 1024).astype(np.float32)
    Wq = np.random.randn(1024, 4096).astype(np.float32) * 0.02
    Wk = np.random.randn(1024, 4096).astype(np.float32) * 0.02
    Wv = np.random.randn(1024, 4096).astype(np.float32) * 0.02
    Wo = np.random.randn(4096, 1024).astype(np.float32) * 0.02
    return {"x": x, "Wq": Wq, "Wk": Wk, "Wv": Wv, "Wo": Wo}

def reference(x, Wq, Wk, Wv, Wo):
    B, Sq, Hq, Dh = 8, 512, 32, 128
    inv = 1.0 / (10000.0 ** (np.arange(0, Dh, 2) / Dh))
    pos = np.arange(Sq)[:, None] * inv[None, :]
    cos = np.repeat(np.cos(pos), 2, axis=-1).astype(np.float32)
    sin = np.repeat(np.sin(pos), 2, axis=-1).astype(np.float32)
    def rot(t):
        t2 = t.reshape(B, Sq, Hq, Dh // 2, 2)
        t_r = np.stack([-t2[..., 1], t2[..., 0]], axis=-1).reshape(B, Sq, Hq, Dh)
        return t * cos[None, :, None, :] + t_r * sin[None, :, None, :]
    Q = rot((x @ Wq).reshape(B, Sq, Hq, Dh))
    K = rot((x @ Wk).reshape(B, Sq, Hq, Dh))
    V = (x @ Wv).reshape(B, Sq, Hq, Dh)
    s = np.einsum('bihd,bjhd->bhij', Q, K).astype(np.float32) * 0.08838834764831843
    s_max = s.max(axis=-1, keepdims=True)
    w = np.exp(s - s_max)
    w = w / w.sum(axis=-1, keepdims=True)
    ctx = np.einsum('bhij,bjhd->bihd', w, V).reshape(B, Sq, Hq * Dh)
    return ctx @ Wo
```

```python
import functools
import math

import jax
import jax.numpy as jnp
from jax import lax
from jax.experimental import pallas as pl
from jax.experimental.pallas import tpu as pltpu

N_DEV = 4
B_LOC = 2
SQ = 512
D = 1024
H_LOC = 8
DH = 128
SCALE = 0.08838834764831843
N_STEPS = N_DEV * B_LOC

_RELS = (-1, 1, 2)
_INV_K = (1, 0, 2)


def _rope_tables():
    lane = lax.broadcasted_iota(jnp.int32, (SQ, DH), 1)
    pos = lax.broadcasted_iota(jnp.int32, (SQ, DH), 0).astype(jnp.float32)
    pair = (lane // 2 * 2).astype(jnp.float32)
    inv = jnp.exp(pair * (-math.log(10000.0) / DH))
    ang = pos * inv
    cos = jnp.cos(ang)
    sin = jnp.sin(ang)
    even = (lane % 2) == 0
    sin_signed = jnp.where(even, -sin, sin)
    return cos, sin_signed, even


def _rope(t, cos, sin_signed, even):
    nxt = pltpu.roll(t, DH - 1, 1)
    prv = pltpu.roll(t, 1, 1)
    swapped = jnp.where(even, nxt, prv)
    return t * cos + swapped * sin_signed


def pallas_dist_rope_attn_htp_bs_b2_sq512_d1024_hq8_dh128_kernel(
    x: jax.Array,
    Wq: jax.Array,
    Wk: jax.Array,
    Wv: jax.Array,
    Wo: jax.Array,
):
    def body(x_hbm, wq_hbm, wk_hbm, wv_hbm, wo_hbm, out_hbm,
             xst, wst, xg, wb, rs_s, rs_r, own, ost, tabs,
             ld_sems, ag_ss, ag_rs, rs_ss, rs_rs, out_sems):
        me = lax.axis_index("i")

        cp_x = [pltpu.make_async_copy(x_hbm.at[b], xst.at[b], ld_sems.at[b])
                for b in range(B_LOC)]
        w_hbm = (wq_hbm, wk_hbm, wv_hbm, wo_hbm)
        cp_w = [pltpu.make_async_copy(w_hbm[i], wst.at[i], ld_sems.at[2 + i])
                for i in range(4)]
        for c in cp_x:
            c.start()
        for c in cp_w:
            c.start()

        own_slot = (0, N_STEPS - 1)

        def ag_copy(b, k):
            tgt = (me + _RELS[k]) % N_DEV
            slot = 1 + _INV_K[k] + 3 * b
            return pltpu.make_async_remote_copy(
                src_ref=xg.at[own_slot[b]],
                dst_ref=xg.at[slot],
                send_sem=ag_ss.at[3 * b + k],
                recv_sem=ag_rs.at[slot - 1],
                device_id=(tgt,),
                device_id_type=pl.DeviceIdType.MESH,
            )

        for b in range(B_LOC):
            cp_x[b].wait()
            xg[own_slot[b]] = xst[b].astype(jnp.bfloat16)
            for k in range(3):
                ag_copy(b, k).start()

        cos, sin_signed, even = _rope_tables()
        tabs[0] = cos
        tabs[1] = sin_signed
        tabs[2] = cos * SCALE
        tabs[3] = sin_signed * SCALE

        for i in range(4):
            cp_w[i].wait()
            wb[i] = wst[i].astype(jnp.bfloat16)

        def step(s, carry):
            is_remote = jnp.logical_and(s >= 1, s <= N_STEPS - 2)

            @pl.when(is_remote)
            def _():
                pltpu.make_async_remote_copy(
                    src_ref=xg.at[s], dst_ref=xg.at[s],
                    send_sem=ag_ss.at[0], recv_sem=ag_rs.at[s - 1],
                    device_id=(me,), device_id_type=pl.DeviceIdType.MESH,
                ).wait_recv()

            xb = xg[s]
            lane = lax.broadcasted_iota(jnp.int32, (SQ, DH), 1)
            even = (lane % 2) == 0
            q = jnp.dot(xb, wb[0], preferred_element_type=jnp.float32)
            k = jnp.dot(xb, wb[1], preferred_element_type=jnp.float32)
            v = jnp.dot(xb, wb[2], preferred_element_type=jnp.float32)
            ctxs = []
            for h in range(H_LOC):
                sl = slice(h * DH, (h + 1) * DH)
                qh = _rope(q[:, sl], tabs[2], tabs[3], even).astype(jnp.bfloat16)
                kh = _rope(k[:, sl], tabs[0], tabs[1], even).astype(jnp.bfloat16)
                vh = v[:, sl].astype(jnp.bfloat16)
                sc = lax.dot_general(qh, kh, (((1,), (1,)), ((), ())),
                                     preferred_element_type=jnp.float32)
                m = jnp.max(sc, axis=-1, keepdims=True)
                p = jnp.exp(sc - m)
                l = jnp.sum(p, axis=-1, keepdims=True)
                c = jnp.dot(p.astype(jnp.bfloat16), vh,
                            preferred_element_type=jnp.float32)
                ctxs.append((c / l).astype(jnp.bfloat16))
            ctx = jnp.concatenate(ctxs, axis=-1)
            part = jnp.dot(ctx, wb[3], preferred_element_type=jnp.float32)

            @pl.when(s == 0)
            def _():
                own[0] = part

            @pl.when(s == N_STEPS - 1)
            def _():
                own[1] = part

            @pl.when(is_remote)
            def _():
                j = s - 1
                kk = j % 3
                b = j // 3
                rel = jnp.where(kk == 0, -1, jnp.where(kk == 1, 1, 2))
                inv_k = jnp.where(kk == 0, 1, jnp.where(kk == 1, 0, 2))
                tgt = (me + rel + N_DEV) % N_DEV
                rslot = inv_k + 3 * b
                rs_s[j] = part.astype(jnp.bfloat16)
                pltpu.make_async_remote_copy(
                    src_ref=rs_s.at[j], dst_ref=rs_r.at[rslot],
                    send_sem=rs_ss.at[j], recv_sem=rs_rs.at[rslot],
                    device_id=(tgt,), device_id_type=pl.DeviceIdType.MESH,
                ).start()

            return carry

        lax.fori_loop(0, N_STEPS, step, 0)

        out_cps = []
        for b in range(B_LOC):
            acc = own[b]
            for k in range(3):
                j = 3 * b + k
                pltpu.make_async_remote_copy(
                    src_ref=rs_s.at[j], dst_ref=rs_r.at[j],
                    send_sem=rs_ss.at[j], recv_sem=rs_rs.at[j],
                    device_id=(me,), device_id_type=pl.DeviceIdType.MESH,
                ).wait_recv()
                acc = acc + rs_r[j].astype(jnp.float32)
            ost[b] = acc
            cp = pltpu.make_async_copy(ost.at[b], out_hbm.at[b], out_sems.at[b])
            cp.start()
            out_cps.append(cp)

        for b in range(B_LOC):
            for k in range(3):
                ag_copy(b, k).wait_send()
        for j in range(6):
            pltpu.make_async_remote_copy(
                src_ref=rs_s.at[j], dst_ref=rs_r.at[j],
                send_sem=rs_ss.at[j], recv_sem=rs_rs.at[j],
                device_id=(me,), device_id_type=pl.DeviceIdType.MESH,
            ).wait_send()
        for cp in out_cps:
            cp.wait()

    any_spec = pl.BlockSpec(memory_space=pl.ANY)
    return pl.pallas_call(
        body,
        out_shape=jax.ShapeDtypeStruct((B_LOC, SQ, D), jnp.float32),
        in_specs=[any_spec] * 5,
        out_specs=any_spec,
        scratch_shapes=[
            pltpu.VMEM((B_LOC, SQ, D), jnp.float32),
            pltpu.VMEM((4, D, D), jnp.float32),
            pltpu.VMEM((N_STEPS, SQ, D), jnp.bfloat16),
            pltpu.VMEM((4, D, D), jnp.bfloat16),
            pltpu.VMEM((6, SQ, D), jnp.bfloat16),
            pltpu.VMEM((6, SQ, D), jnp.bfloat16),
            pltpu.VMEM((B_LOC, SQ, D), jnp.float32),
            pltpu.VMEM((B_LOC, SQ, D), jnp.float32),
            pltpu.VMEM((4, SQ, DH), jnp.float32),
            pltpu.SemaphoreType.DMA((6,)),
            pltpu.SemaphoreType.DMA((6,)),
            pltpu.SemaphoreType.DMA((6,)),
            pltpu.SemaphoreType.DMA((6,)),
            pltpu.SemaphoreType.DMA((6,)),
            pltpu.SemaphoreType.DMA((2,)),
        ],
        compiler_params=pltpu.CompilerParams(
            vmem_limit_bytes=100 * 1024 * 1024,
        ),
    )(x, Wq, Wk, Wv, Wo)
```

```python
import math

import jax
import jax.numpy as jnp
from jax import lax
from jax.experimental import pallas as pl
from jax.experimental.pallas import tpu as pltpu

N_DEV = 4
B_LOC = 2
SQ = 512
D = 1024
H_LOC = 8
DH = 128
SCALE = 0.08838834764831843
N_STEPS = N_DEV * B_LOC
N_GRP = 4
GW = D // N_GRP

_RELS = (-1, 1, 2)
_INV_K = (1, 0, 2)


def _rope_tables():
    lane = lax.broadcasted_iota(jnp.int32, (SQ, DH), 1)
    pos = lax.broadcasted_iota(jnp.int32, (SQ, DH), 0).astype(jnp.float32)
    pair = (lane // 2 * 2).astype(jnp.float32)
    inv = jnp.exp(pair * (-math.log(10000.0) / DH))
    ang = pos * inv
    cos = jnp.cos(ang)
    sin = jnp.sin(ang)
    even = (lane % 2) == 0
    sin_signed = jnp.where(even, -sin, sin)
    return cos, sin_signed


def _rope(t, cos, sin_signed, even):
    nxt = pltpu.roll(t, DH - 1, 1)
    prv = pltpu.roll(t, 1, 1)
    swapped = jnp.where(even, nxt, prv)
    return t * cos + swapped * sin_signed


def _attn_heads(q, k, v, tabs, n_heads):
    lane = lax.broadcasted_iota(jnp.int32, (SQ, DH), 1)
    even = (lane % 2) == 0
    ctxs = []
    for h in range(n_heads):
        sl = slice(h * DH, (h + 1) * DH)
        qh = _rope(q[:, sl], tabs[2], tabs[3], even).astype(jnp.bfloat16)
        kh = _rope(k[:, sl], tabs[0], tabs[1], even).astype(jnp.bfloat16)
        vh = v[:, sl].astype(jnp.bfloat16)
        sc = lax.dot_general(qh, kh, (((1,), (1,)), ((), ())),
                             preferred_element_type=jnp.float32)
        m = jnp.max(sc, axis=-1, keepdims=True)
        p = jnp.exp(sc - m)
        l = jnp.sum(p, axis=-1, keepdims=True)
        c = jnp.dot(p.astype(jnp.bfloat16), vh,
                    preferred_element_type=jnp.float32)
        ctxs.append((c / l).astype(jnp.bfloat16))
    return ctxs


def pallas_dist_rope_attn_htp_bs_b2_sq512_d1024_hq8_dh128_kernel(
    x: jax.Array,
    Wq: jax.Array,
    Wk: jax.Array,
    Wv: jax.Array,
    Wo: jax.Array,
):
    def body(x_hbm, wq_hbm, wk_hbm, wv_hbm, wo_hbm, out_ref,
             xst, wst, xg, wb, rs_s, rs_r, tabs,
             ld_sems, ag_ss, ag_rs, rs_ss, rs_rs):
        me = lax.axis_index("i")
        own_slot = (0, N_STEPS - 1)

        cp_x = [pltpu.make_async_copy(x_hbm.at[b], xst.at[b], ld_sems.at[b])
                for b in range(B_LOC)]
        qkv_hbm = (wq_hbm, wk_hbm, wv_hbm)

        def cp_g(g, i):
            return pltpu.make_async_copy(
                qkv_hbm[i].at[:, pl.ds(g * GW, GW)],
                wst.at[i, :, pl.ds(g * GW, GW)],
                ld_sems.at[3 + 3 * g + i])

        cp_wo = pltpu.make_async_copy(wo_hbm, wst.at[3], ld_sems.at[2])

        def ag_copy(b, k):
            tgt = (me + _RELS[k] + N_DEV) % N_DEV
            slot = 1 + _INV_K[k] + 3 * b
            return pltpu.make_async_remote_copy(
                src_ref=xg.at[own_slot[b]],
                dst_ref=xg.at[slot],
                send_sem=ag_ss.at[3 * b + k],
                recv_sem=ag_rs.at[slot - 1],
                device_id=(tgt,),
                device_id_type=pl.DeviceIdType.MESH,
            )

        with jax.named_scope("step0"):
            cp_x[0].start()

            cos, sin_signed = _rope_tables()
            tabs[0] = cos
            tabs[1] = sin_signed
            tabs[2] = cos * SCALE
            tabs[3] = sin_signed * SCALE

            cp_x[0].wait()
            for g in range(2):
                for i in range(3):
                    cp_g(g, i).start()
            xg[0] = xst[0].astype(jnp.bfloat16)
            ag_copy(0, 0).start()
            ag_copy(0, 1).start()

            ctxs = []
            for g in range(N_GRP):
                cs = slice(g * GW, (g + 1) * GW)
                for i in range(3):
                    cp_g(g, i).wait()
                    wb[i, :, cs] = wst[i, :, cs].astype(jnp.bfloat16)
                if g + 2 < N_GRP:
                    for i in range(3):
                        cp_g(g + 2, i).start()
                elif g + 2 == N_GRP:
                    cp_x[1].start()
                    cp_wo.start()
                xb = xg[0]
                q = jnp.dot(xb, wb[0, :, cs], preferred_element_type=jnp.float32)
                k = jnp.dot(xb, wb[1, :, cs], preferred_element_type=jnp.float32)
                v = jnp.dot(xb, wb[2, :, cs], preferred_element_type=jnp.float32)
                ctxs += _attn_heads(q, k, v, tabs, GW // DH)

            cp_x[1].wait()
            xg[N_STEPS - 1] = xst[1].astype(jnp.bfloat16)

            cp_wo.wait()
            wb[3] = wst[3].astype(jnp.bfloat16)
            ctx = jnp.concatenate(ctxs, axis=-1)
            out_ref[0] = jnp.dot(ctx, wb[3], preferred_element_type=jnp.float32)

        def step(s, carry):
            is_remote = s <= N_STEPS - 2

            @pl.when(is_remote)
            def _():
                with jax.named_scope("ag_wait"):
                    pltpu.make_async_remote_copy(
                        src_ref=xg.at[s], dst_ref=xg.at[s],
                        send_sem=ag_ss.at[0], recv_sem=ag_rs.at[s - 1],
                        device_id=(me,), device_id_type=pl.DeviceIdType.MESH,
                    ).wait_recv()

            @pl.when(s == 1)
            def _():
                ag_copy(0, 2).start()
                for k in range(3):
                    ag_copy(1, k).start()

            xb = xg[s]
            q = jnp.dot(xb, wb[0], preferred_element_type=jnp.float32)
            k = jnp.dot(xb, wb[1], preferred_element_type=jnp.float32)
            v = jnp.dot(xb, wb[2], preferred_element_type=jnp.float32)
            ctx = jnp.concatenate(_attn_heads(q, k, v, tabs, H_LOC), axis=-1)
            part = jnp.dot(ctx, wb[3], preferred_element_type=jnp.float32)

            @pl.when(s == N_STEPS - 1)
            def _():
                out_ref[1] = part

            @pl.when(is_remote)
            def _():
                j = s - 1
                kk = j % 3
                b = j // 3
                rel = jnp.where(kk == 0, -1, jnp.where(kk == 1, 1, 2))
                inv_k = jnp.where(kk == 0, 1, jnp.where(kk == 1, 0, 2))
                tgt = (me + rel + N_DEV) % N_DEV
                rslot = inv_k + 3 * b
                rs_s[j] = part.astype(jnp.bfloat16)
                with jax.named_scope("rs_send"):
                    pltpu.make_async_remote_copy(
                        src_ref=rs_s.at[j], dst_ref=rs_r.at[rslot],
                        send_sem=rs_ss.at[j], recv_sem=rs_rs.at[rslot],
                        device_id=(tgt,), device_id_type=pl.DeviceIdType.MESH,
                    ).start()

            return carry

        with jax.named_scope("loop"):
            lax.fori_loop(1, N_STEPS, step, 0)

        with jax.named_scope("final"):
            for b in range(B_LOC):
                acc = out_ref[b]
                for k in range(3):
                    j = 3 * b + k
                    pltpu.make_async_remote_copy(
                        src_ref=rs_s.at[j], dst_ref=rs_r.at[j],
                        send_sem=rs_ss.at[j], recv_sem=rs_rs.at[j],
                        device_id=(me,), device_id_type=pl.DeviceIdType.MESH,
                    ).wait_recv()
                    acc = acc + rs_r[j].astype(jnp.float32)
                out_ref[b] = acc

            for b in range(B_LOC):
                for k in range(3):
                    ag_copy(b, k).wait_send()
            for j in range(6):
                pltpu.make_async_remote_copy(
                    src_ref=rs_s.at[j], dst_ref=rs_r.at[j],
                    send_sem=rs_ss.at[j], recv_sem=rs_rs.at[j],
                    device_id=(me,), device_id_type=pl.DeviceIdType.MESH,
                ).wait_send()

    hbm_spec = pl.BlockSpec(memory_space=pltpu.HBM)
    return pl.pallas_call(
        body,
        out_shape=jax.ShapeDtypeStruct((B_LOC, SQ, D), jnp.float32),
        in_specs=[hbm_spec] * 5,
        out_specs=pl.BlockSpec(memory_space=pltpu.VMEM),
        scratch_shapes=[
            pltpu.VMEM((B_LOC, SQ, D), jnp.float32),
            pltpu.VMEM((4, D, D), jnp.float32),
            pltpu.VMEM((N_STEPS, SQ, D), jnp.bfloat16),
            pltpu.VMEM((4, D, D), jnp.bfloat16),
            pltpu.VMEM((6, SQ, D), jnp.bfloat16),
            pltpu.VMEM((6, SQ, D), jnp.bfloat16),
            pltpu.VMEM((4, SQ, DH), jnp.float32),
            pltpu.SemaphoreType.DMA((3 + 3 * N_GRP,)),
            pltpu.SemaphoreType.DMA((6,)),
            pltpu.SemaphoreType.DMA((6,)),
            pltpu.SemaphoreType.DMA((6,)),
            pltpu.SemaphoreType.DMA((6,)),
        ],
        compiler_params=pltpu.CompilerParams(
            vmem_limit_bytes=100 * 1024 * 1024,
        ),
    )(x, Wq, Wk, Wv, Wo)
```
